```python
import numpy as np
kernel_name = 'dist_attn_self_mha_htp_b1_sq256_skv256_d1024_hq8_dh128'

def setup_inputs():
    x = np.random.randn(1, 256, 1024).astype(np.float32)
    Wq = np.random.randn(1024, 4096).astype(np.float32) * 0.02
    Wk = np.random.randn(1024, 4096).astype(np.float32) * 0.02
    Wv = np.random.randn(1024, 4096).astype(np.float32) * 0.02
    Wo = np.random.randn(4096, 1024).astype(np.float32) * 0.02
    return {'x': x, 'Wq': Wq, 'Wk': Wk, 'Wv': Wv, 'Wo': Wo}

def reference(x, Wq, Wk, Wv, Wo):
    B, Sq, Hq, Hkv, Dh = (1, 256, 32, 32, 128)
    Q = (x @ Wq).reshape(B, Sq, Hq, Dh)
    K = (x @ Wk).reshape(B, Sq, Hkv, Dh)
    V = (x @ Wv).reshape(B, Sq, Hkv, Dh)
    Skv = K.shape[1]
    out = np.zeros((B, Sq, Hq, Dh), dtype=np.float32)
    m = np.full((B, Hq, Sq, 1), -np.inf, dtype=np.float32)
    l = np.zeros((B, Hq, Sq, 1), dtype=np.float32)
    for j0 in range(0, Skv, 256):
        Kj = K[:, j0:j0 + 256].copy()
        Vj = V[:, j0:j0 + 256].copy()
        sj = np.einsum('bihd,bjhd->bhij', Q, Kj).astype(np.float32) * 0.08838834764831843
        mj = sj.max(axis=-1, keepdims=True)
        m_new = np.maximum(m, mj)
        alpha = np.exp(m - m_new)
        pj = np.exp(sj - m_new)
        l = l * alpha + pj.sum(axis=-1, keepdims=True)
        out = out * alpha.transpose(0, 2, 1, 3) + np.einsum('bhij,bjhd->bihd', pj, Vj)
        m = m_new
    out = (out / l.transpose(0, 2, 1, 3)).reshape(B, Sq, Hq * Dh)
    return out @ Wo
```

```python
import contextlib
import jax, jax.numpy as jnp
from jax import lax
from jax.experimental import pallas as pl
from jax.experimental.pallas import tpu as pltpu

F32 = jnp.float32; BF = jnp.bfloat16
SCALE = 0.08838834764831843
MESH = pl.DeviceIdType.MESH
NT = (((1,), (1,)), ((), ()))

def make(scoped=False, semcheck=False, pq="xxyy", MR=128):
    scope = (lambda n: jax.named_scope(n)) if scoped else (lambda n: contextlib.nullcontext())
    NM = 256 // MR
    def fn(x, Wq, Wk, Wv, Wo):
        def body(x_hbm, wq_hbm, wk_hbm, wv_hbm, wo_hbm, out_ref,
                 xf, wq, wk, wv, wo, xb, qb, kb, vb, pb, ab,
                 s1, r1, acc, s2, r2, s3, r3, lsem, ssem, rsem):
            me = lax.axis_index("i")
            bbit = me // 2
            abit = (me % 2) ^ bbit
            bar = pltpu.get_barrier_semaphore()
            nbx = me ^ 1
            nby = me ^ 3
            if pq == "xxyy":
                cP = bbit
            elif pq == "xxxx":
                cP = bbit * 0
            elif pq == "xxxy":
                cP = (me == 3).astype(jnp.int32)
            col = {"P": cP, "Q": 1 - cP}
            nb = {c: jnp.where(col[c] == 0, nbx, nby) for c in "PQ"}
            keep = {c: jnp.where(col[c] == 0, abit, bbit) for c in "PQ"}
            other = {"P": "Q", "Q": "P"}
            def blk(c, role, n):
                return 4 * col[c] + 2 * (keep[c] if role == "K" else 1 - keep[c]) + n
            order = [("P","S",0), ("Q","S",0), ("P","S",1), ("Q","S",1), ("Q","K",0), ("P","K",0), ("Q","K",1), ("P","K",1)]

            cps = {}
            n = [0]
            def ld(name, src, dst):
                cp = pltpu.make_async_copy(src, dst, lsem.at[n[0]]); n[0] += 1
                cp.start(); cps.setdefault(name, []).append(cp)
            ld("x", x_hbm.at[0], xf)
            for g in range(2):
                ld(f"q{g}", wq_hbm.at[:, pl.ds(g*512, 512)], wq.at[g])
                if g == 0:
                    ld(f"k{g}", wk_hbm.at[:, pl.ds(g*512, 512)], wk.at[g])
                else:
                    for hf in range(2):
                        ld(f"k{g}{hf}", wk_hbm.at[pl.ds(hf*512, 512), pl.ds(g*512, 512)], wk.at[g, pl.ds(hf*512, 512)])
            for h in range(8):
                for hf in range(2):
                    ld(f"v{h}", wv_hbm.at[:, hf, :, pl.ds(h*128, 128)], wv.at[h, :, hf])
            for k, (c, role, nn) in enumerate(order):
                c0 = pl.multiple_of(blk(c, role, nn) * 128, 128)
                for hf in range(2):
                    ld(f"o{k}", wo_hbm.at[:, hf, :, pl.ds(c0, 128)], wo.at[k, :, hf])

            for d in (nbx, nby):
                pl.semaphore_signal(bar, inc=1, device_id=(d,), device_id_type=MESH)

            def wait(name):
                with scope("wait_" + name):
                    for cp in cps[name]: cp.wait()

            def softmax(h):
                g, hh = divmod(h, 4)
                s = lax.dot_general(qb[g, :, hh*128:(hh+1)*128], kb[g, :, hh*128:(hh+1)*128], NT, preferred_element_type=F32)
                m = jnp.max(s, axis=-1, keepdims=True)
                e = jnp.exp(s - m)
                l = jnp.sum(e, axis=-1, keepdims=True)
                pb[h] = (e * (1.0 / l)).astype(BF)
            def pv(h):
                ab[:, h*128:(h+1)*128] = jnp.dot(pb[h], vb[h], preferred_element_type=F32).astype(BF)

            wait("x")
            with scope("cvt_x"):
                xb[...] = xf[...].astype(BF)
            wait("q0")
            with scope("mm_q0"):
                qb[0] = (jnp.dot(xb[...], wq[0].astype(BF), preferred_element_type=F32) * SCALE).astype(BF)
            wait("k0")
            with scope("mm_k0"):
                kb[0] = jnp.dot(xb[...], wk[0].astype(BF), preferred_element_type=F32).astype(BF)
                for h in range(4): softmax(h)
            wait("q1")
            with scope("mm_q1"):
                qb[1] = (jnp.dot(xb[...], wq[1].astype(BF), preferred_element_type=F32) * SCALE).astype(BF)
            pl.semaphore_wait(bar, 2)
            wait("k10")
            with scope("mm_k10"):
                xf[:, 0:512] = jnp.dot(xb[:, 0:512], wk[1, 0:512].astype(BF), preferred_element_type=F32)
            wait("k11")
            with scope("mm_k11"):
                kb[1] = (xf[:, 0:512] + jnp.dot(xb[:, 512:], wk[1, 512:].astype(BF), preferred_element_type=F32)).astype(BF)
            for h in range(8):
                wait(f"v{h}")
                with scope(f"mm_v{h}"):
                    vb[h] = jnp.dot(xb[...], wv[h].reshape(1024, 128).astype(BF), preferred_element_type=F32).astype(BF)
                    if h < 4: softmax(4 + h)
                    if h > 0: pv(h - 1)
                    if h == 7: pv(7)

            sends = []
            def rdma(src, dst, step, c, nn, m, dev):
                idx = ((step * 2 + col[c]) * 2 + nn) * NM + m
                slot = col[c] * 2 + nn
                rows = pl.ds(m * MR, MR)
                return pltpu.make_async_remote_copy(src.at[slot, rows], dst.at[slot, rows], ssem.at[idx], rsem.at[idx],
                                                    device_id=(dev,), device_id_type=MESH)
            for k, (c, role, nn) in enumerate(order):
                wait(f"o{k}")
                slot = col[c] * 2 + nn
                for hf in range(2):
                    rows = pl.ds(hf * 128, 128)
                    ms = range(hf * NM // 2, (hf + 1) * NM // 2)
                    if role == "K":
                        with scope(f"wr1_{k}{hf}"):
                            for m in ms: rdma(s1, r1, 0, c, nn, m, nb[c]).wait_recv()
                    with scope(f"mm_o{k}{hf}"):
                        part = jnp.dot(ab[rows, :], wo[k].reshape(1024, 128).astype(BF), preferred_element_type=F32)
                        if role == "S":
                            s1[slot, rows] = part.astype(BF)
                            for m in ms:
                                cp = rdma(s1, r1, 0, c, nn, m, nb[c]); cp.start(); sends.append(cp)
                        else:
                            pair = part + r1[slot, rows].astype(F32)
                            acc[slot, rows] = pair
                            s2[slot, rows] = pair.astype(BF)
                            for m in ms:
                                cp = rdma(s2, r2, 1, c, nn, m, nb[other[c]]); cp.start(); sends.append(cp)
            for nn in range(2):
                for m in range(NM):
                    for c in "QP":
                        slot = col[c] * 2 + nn
                        rows = pl.ds(m * MR, MR)
                        with scope(f"wr2_{nn}{m}{c}"):
                            rdma(s2, r2, 1, c, nn, m, nb[other[c]]).wait_recv()
                        fin = acc[slot, rows] + r2[slot, rows].astype(F32)
                        s3[slot, rows] = fin.astype(BF)
                        cp = rdma(s3, r3, 2, c, nn, m, nb[c]); cp.start(); sends.append(cp)
                        c0 = pl.multiple_of(blk(c, "K", nn) * 128, 128)
                        out_ref[0, rows, pl.ds(c0, 128)] = fin
            for nn in range(2):
                for m in range(NM):
                    for c in "QP":
                        slot = col[c] * 2 + nn
                        rows = pl.ds(m * MR, MR)
                        with scope(f"wr3_{nn}{m}{c}"):
                            rdma(s3, r3, 2, c, nn, m, nb[c]).wait_recv()
                        c0 = pl.multiple_of(blk(c, "S", nn) * 128, 128)
                        out_ref[0, rows, pl.ds(c0, 128)] = r3[slot, rows].astype(F32)
            with scope("wsend"):
                for cp in sends: cp.wait_send()

        ANY = pl.BlockSpec(memory_space=pl.ANY)
        V = pltpu.VMEM
        cb = lambda dt: V((4, 256, 128), dt)
        return pl.pallas_call(body, out_shape=jax.ShapeDtypeStruct(x.shape, F32),
            in_specs=[ANY]*5, out_specs=pl.BlockSpec(memory_space=pltpu.VMEM),
            scratch_shapes=[V((256, 1024), F32), V((2, 1024, 512), F32), V((2, 1024, 512), F32),
                            V((8, 32, 2, 16, 128), F32), V((8, 32, 2, 16, 128), F32),
                            V((256, 1024), BF), V((2, 256, 512), BF), V((2, 256, 512), BF), V((8, 256, 128), BF),
                            V((8, 256, 256), BF), V((256, 1024), BF),
                            cb(BF), cb(BF), cb(F32), cb(BF), cb(BF), cb(BF), cb(BF),
                            pltpu.SemaphoreType.DMA((38,)), pltpu.SemaphoreType.DMA((12*NM,)), pltpu.SemaphoreType.DMA((12*NM,))],
            compiler_params=pltpu.CompilerParams(collective_id=0, vmem_limit_bytes=64*1024*1024,
                                                 disable_semaphore_checks=not semcheck, disable_bounds_checks=not semcheck),
        )(x, Wq, Wk, Wv.reshape(32, 2, 16, 1024), Wo.reshape(32, 2, 16, 1024))
    return fn


_impl = make()


def pallas_dist_attn_self_mha_htp_b1_sq256_skv256_d1024_hq8_dh128_kernel(x, Wq, Wk, Wv, Wo):
    return _impl(x, Wq, Wk, Wv, Wo)
```

```python
import contextlib
import jax, jax.numpy as jnp
from jax import lax
from jax.experimental import pallas as pl
from jax.experimental.pallas import tpu as pltpu

F32 = jnp.float32; BF = jnp.bfloat16
SCALE = 0.08838834764831843
MESH = pl.DeviceIdType.MESH
NT = (((1,), (1,)), ((), ()))

def default_prog(MR=64, first64=False):
    NM = 128 // MR
    ms = lambda h: range(h * NM, (h + 1) * NM)
    p = []
    for n in range(2):
        for c in "PQ":
            for h in range(2):
                if first64 and n == 0 and c == "P" and h == 0:
                    p += [("mm", c, "S", n, 0, 64), ("s1", c, n, 0), ("mm", c, "S", n, 64, 64), ("s1", c, n, 1)]
                else:
                    p += [("mm", c, "S", n, h * 128, 128)] + [("s1", c, n, m) for m in ms(h)]
    if NM == 1:
        for n in range(2):
            p += [("mm", "Q", "K", n, 0, 128), ("s2", "Q", n, 0), ("mm", "Q", "K", n, 128, 128), ("mm", "P", "K", n, 0, 128),
                  ("s2", "P", n, 0), ("s2", "Q", n, 1), ("mm", "P", "K", n, 128, 128), ("s2", "P", n, 1)]
    else:
        for n in range(2):
            p += [("mm", "Q", "K", n, 0, 128), ("s2", "Q", n, 0), ("mm", "Q", "K", n, 128, 128), ("s2", "Q", n, 1),
                  ("mm", "P", "K", n, 0, 128), ("s2", "P", n, 0), ("s2", "P", n, 1), ("s2", "Q", n, 2),
                  ("mm", "P", "K", n, 128, 128), ("s2", "P", n, 2), ("s2", "P", n, 3), ("s2", "Q", n, 3)]
    for n in range(2):
        for m in range(2 * NM):
            p += [("s3", "Q", n, m), ("s3", "P", n, m)]
    for n in range(2):
        for m in range(2 * NM):
            p += [("fin", "P", n, m), ("fin", "Q", n, m)]
    return p

def make(scoped=False, semcheck=False, pq="xxyy", prog=None, MR=64, first64=False, pvsplit=True, sm0early=False):
    scope = (lambda n: jax.named_scope(n)) if scoped else (lambda n: contextlib.nullcontext())
    prog = prog or default_prog(MR, first64)
    NMB = 256 // MR
    order = []
    for op in prog:
        if op[0] == "mm" and op[1:4] not in order: order.append(op[1:4])
    def fn(x, Wq, Wk, Wv, Wo):
        def body(x_hbm, wq_hbm, wk_hbm, wv_hbm, wo_hbm, out_ref,
                 xf, wq, wk0, wk1, wv, wo, xb, qb, kb, vb, pb, ab,
                 s1, r1, acc, s2, r2, s3, r3, lsem, ssem, rsem, xssem, xrsem):
            me = lax.axis_index("i")
            bbit = me // 2
            abit = (me % 2) ^ bbit
            bar = pltpu.get_barrier_semaphore()
            nbx = me ^ 1
            nby = me ^ 3
            dia = me ^ 2

            cps = {}
            n = [0]
            def ld(name, src, dst):
                cp = pltpu.make_async_copy(src, dst, lsem.at[n[0]]); n[0] += 1
                cp.start(); cps.setdefault(name, []).append(cp)
            ld("x", x_hbm.at[0, pl.ds(pl.multiple_of(me * 64, 64), 64)], xf)
            ld("q0", wq_hbm.at[:, pl.ds(0, 512)], wq.at[0])
            for d in (nbx, nby):
                pl.semaphore_signal(bar, inc=1, device_id=(d,), device_id_type=MESH)
            ld("k0", wk_hbm.at[:, :, :, pl.ds(0, 512)], wk0)
            ld("q1", wq_hbm.at[:, pl.ds(512, 512)], wq.at[1])
            for h in range(4, 8):
                for hf in range(2):
                    ld(f"k{h}", wk_hbm.at[:, hf, :, pl.ds(h*128, 128)], wk1.at[(h - 4) // 2, :, hf, :, pl.ds((h % 2) * 128, 128)])

            cP = {"xxyy": bbit, "xxxx": bbit * 0, "xxxy": (me == 3).astype(jnp.int32), "yxxy": 1 - abit,
                  "yxyy": (me != 1).astype(jnp.int32)}[pq]
            col = {"P": cP, "Q": 1 - cP}
            nb = {c: jnp.where(col[c] == 0, nbx, nby) for c in "PQ"}
            keep = {c: jnp.where(col[c] == 0, abit, bbit) for c in "PQ"}
            other = {"P": "Q", "Q": "P"}
            def blk(c, role, n):
                return 4 * col[c] + 2 * (keep[c] if role == "K" else 1 - keep[c]) + n
            def late_loads():
                for h in range(8):
                    for hf in range(2):
                        ld(f"v{h}", wv_hbm.at[:, hf, :, pl.ds(h*128, 128)], wv.at[h // 2, :, hf, :, pl.ds((h % 2) * 128, 128)])
                for k, (c, role, nn) in enumerate(order):
                    c0 = pl.multiple_of(blk(c, role, nn) * 128, 128)
                    for hf in range(2):
                        ld(f"o{k}", wo_hbm.at[:, hf, :, pl.ds(c0, 128)], wo.at[k, :, hf])

            def wait(*names):
                with scope("wait_" + names[-1]):
                    for name in names:
                        for cp in cps[name]: cp.wait()

            al = slice(None)
            def softmax(h):
                s = lax.dot_general(qb[:, h*128:(h+1)*128], kb[:, h*128:(h+1)*128], NT, preferred_element_type=F32)
                m = jnp.max(s, axis=-1, keepdims=True)
                e = jnp.exp(s - m)
                l = jnp.sum(e, axis=-1, keepdims=True)
                pb[h] = (e * (1.0 / l)).astype(BF)
            def pv(h, rows=al):
                ab[rows, h*128:(h+1)*128] = jnp.dot(pb[h, rows, :], vb[:, h*128:(h+1)*128], preferred_element_type=F32).astype(BF)
            def proj(dst, w, rows, c0, scale=None):
                r = jnp.dot(xb[rows, :], w.astype(BF), preferred_element_type=F32)
                if scale is not None: r = r * scale
                dst[rows, c0:c0 + w.shape[1]] = r.astype(BF)

            sends = []
            wait("x")
            def xr(q, hf): return pl.ds(pl.multiple_of(q * 64 + hf * 32, 32), 32)
            def xc(q, hf, sem, dev):
                return pltpu.make_async_remote_copy(xb.at[xr(q, hf)], xb.at[xr(q, hf)], xssem.at[sem], xrsem.at[sem],
                                                    device_id=(dev,), device_id_type=MESH)
            with scope("cvt_x"):
                xb[pl.ds(pl.multiple_of(me * 64, 64), 64), :] = xf[...].astype(BF)
            with scope("bar"):
                pl.semaphore_wait(bar, 2)
            for q, hf, sem, dev in ((me, 0, 0, nbx), (me, 1, 2, nby), (me, 1, 1, nbx), (me, 0, 3, nby)):
                cp = xc(q, hf, sem, dev); cp.start(); sends.append(cp)
            with scope("xw0"):
                xc(nbx, 0, 0, nbx).wait_recv()
            cp = xc(nbx, 0, 4, nby); cp.start(); sends.append(cp)
            with scope("xw2"):
                xc(nby, 1, 2, nby).wait_recv()
            cp = xc(nby, 1, 5, nbx); cp.start(); sends.append(cp)
            late_loads()
            near = pl.ds(pl.multiple_of(bbit * 128, 128), 128)
            far = pl.ds(pl.multiple_of((1 - bbit) * 128, 128), 128)
            wait("q0")
            with scope("xw1"):
                xc(nbx, 1, 1, nbx).wait_recv()
            with scope("mm_q0n"):
                proj(qb, wq[0], near, 0, SCALE)
            wait("k0")
            with scope("mm_k0n"):
                proj(kb, wk0[...].reshape(1024, 512), near, 0)
            with scope("xw345"):
                xc(nby, 0, 3, nby).wait_recv()
                xc(dia, 0, 4, nby).wait_recv()
                xc(dia, 1, 5, nbx).wait_recv()
            with scope("mm_qk0f"):
                proj(qb, wq[0], far, 0, SCALE)
                proj(kb, wk0[...].reshape(1024, 512), far, 0)
                if sm0early:
                    for h in range(4): softmax(h)
            for cp in sends: cp.wait_send()
            sends = []
            wait("q1")
            with scope("mm_q1"):
                if not sm0early:
                    for h in range(4): softmax(h)
                proj(qb, wq[1], al, 512, SCALE)
            wait("k4", "k5")
            with scope("mm_k45"):
                proj(kb, wk1[0].reshape(1024, 256), al, 512)
            wait("k6", "k7")
            with scope("mm_k67"):
                softmax(4); softmax(5)
                proj(kb, wk1[1].reshape(1024, 256), al, 768)
            wait("v0", "v1")
            with scope("mm_v01"):
                softmax(6); softmax(7)
                proj(vb, wv[0].reshape(1024, 256), al, 0)
            wait("v2", "v3")
            with scope("mm_v23"):
                pv(0); pv(1)
                proj(vb, wv[1].reshape(1024, 256), al, 256)
            for h in range(4, 8):
                wait(f"v{h}")
                with scope(f"mm_v{h}"):
                    if h % 2 == 0:
                        pv(h - 2); pv(h - 1)
                    proj(vb, wv[h // 2, :, :, :, (h % 2)*128:(h % 2 + 1)*128].reshape(1024, 128), al, 128*h)
                    if h == 7:
                        rr = slice(0, 128) if pvsplit else al
                        pv(6, rr); pv(7, rr)

            def rdma(step, c, nn, m):
                src, dst, dev = ((s1, r1, nb[c]), (s2, r2, nb[other[c]]), (s3, r3, nb[c]))[step]
                slot = col[c] * 2 + nn
                idx = (step * 4 + slot) * NMB + m
                rows = pl.ds(m * MR, MR)
                return pltpu.make_async_remote_copy(src.at[slot, rows], dst.at[slot, rows], ssem.at[idx], rsem.at[idx],
                                                    device_id=(dev,), device_id_type=MESH)
            waited = set()
            nfin = 0
            pv_pending = pvsplit
            for op in prog:
                if op[0] == "mm":
                    _, c, role, nn, r0, nr = op
                    k = order.index((c, role, nn))
                    if k not in waited:
                        wait(f"o{k}"); waited.add(k)
                    slot = col[c] * 2 + nn
                    rows = pl.ds(r0, nr)
                    with scope(f"mm_{c}{role}{nn}_{r0}"):
                        if pv_pending and r0 + nr > 128:
                            pv(6, slice(128, 256)); pv(7, slice(128, 256)); pv_pending = False
                        part = jnp.dot(ab[rows, :], wo[k].reshape(1024, 128).astype(BF), preferred_element_type=F32)
                        if role == "S": s1[slot, rows] = part.astype(BF)
                        else: acc[slot, rows] = part
                    continue
                _, c, nn, m = op
                slot = col[c] * 2 + nn
                rows = pl.ds(m * MR, MR)
                if op[0] == "s1":
                    cp = rdma(0, c, nn, m); cp.start(); sends.append(cp)
                elif op[0] == "s2":
                    with scope(f"s2_{c}{nn}{m}"):
                        rdma(0, c, nn, m).wait_recv()
                    pair = acc[slot, rows] + r1[slot, rows].astype(F32)
                    s2[slot, rows] = pair.astype(BF)
                    cp = rdma(1, c, nn, m); cp.start(); sends.append(cp)
                    acc[slot, rows] = pair
                elif op[0] == "s3":
                    with scope(f"s3_{c}{nn}{m}"):
                        rdma(1, c, nn, m).wait_recv()
                    fin = acc[slot, rows] + r2[slot, rows].astype(F32)
                    s3[slot, rows] = fin.astype(BF)
                    cp = rdma(2, c, nn, m); cp.start(); sends.append(cp)
                    c0 = pl.multiple_of(blk(c, "K", nn) * 128, 128)
                    out_ref[0, rows, pl.ds(c0, 128)] = fin
                else:
                    nfin += 1
                    if nfin == 1:
                        with scope("wsend0"):
                            for cp in sends[:8 * NMB]: cp.wait_send()
                        sends = sends[8 * NMB:]
                    if nfin == 4 * NMB - 1:
                        with scope("wsend1"):
                            for cp in sends[:-2]: cp.wait_send()
                        sends = sends[-2:]
                    with scope(f"fin_{c}{nn}{m}"):
                        rdma(2, c, nn, m).wait_recv()
                    c0 = pl.multiple_of(blk(c, "S", nn) * 128, 128)
                    out_ref[0, rows, pl.ds(c0, 128)] = r3[slot, rows].astype(F32)
            with scope("wsend"):
                for cp in sends: cp.wait_send()

        ANY = pl.BlockSpec(memory_space=pl.ANY)
        V = pltpu.VMEM
        cb = lambda dt: V((4, 256, 128), dt)
        r4 = lambda w: w.reshape(32, 2, 16, 1024)
        return pl.pallas_call(body, out_shape=jax.ShapeDtypeStruct(x.shape, F32),
            in_specs=[ANY]*5, out_specs=pl.BlockSpec(memory_space=pltpu.VMEM),
            scratch_shapes=[V((64, 1024), F32), V((2, 1024, 512), F32), V((32, 2, 16, 512), F32), V((2, 32, 2, 16, 256), F32),
                            V((4, 32, 2, 16, 256), F32), V((8, 32, 2, 16, 128), F32),
                            V((256, 1024), BF), V((256, 1024), BF), V((256, 1024), BF), V((256, 1024), BF),
                            V((8, 256, 256), BF), V((256, 1024), BF),
                            cb(BF), cb(BF), cb(F32), cb(BF), cb(BF), cb(BF), cb(BF),
                            pltpu.SemaphoreType.DMA((44,)), pltpu.SemaphoreType.DMA((12 * NMB,)), pltpu.SemaphoreType.DMA((12 * NMB,)),
                            pltpu.SemaphoreType.DMA((6,)), pltpu.SemaphoreType.DMA((6,))],
            compiler_params=pltpu.CompilerParams(collective_id=0, vmem_limit_bytes=64*1024*1024,
                                                 disable_semaphore_checks=not semcheck, disable_bounds_checks=not semcheck),
        )(x, Wq, r4(Wk), r4(Wv), r4(Wo))
    return fn


_impl = make()


def pallas_dist_attn_self_mha_htp_b1_sq256_skv256_d1024_hq8_dh128_kernel(x, Wq, Wk, Wv, Wo):
    return _impl(x, Wq, Wk, Wv, Wo)
```

```python
import functools

import jax
import jax.numpy as jnp
from jax import lax
from jax.experimental import pallas as pl
from jax.experimental.pallas import tpu as pltpu

F32 = jnp.float32
BF16 = jnp.bfloat16
MESH = pl.DeviceIdType.MESH
SCALE = 0.08838834764831843
N_DEV = 4
SEQ, D, DH = 256, 1024, 128
PIECE = 16
UNITS = 4
ALL = slice(None)

_LOADS = [('q', 0, 3), ('k', 0, 3), ('q', 3, 3), ('k', 3, 3), ('q', 6, 2), ('k', 6, 2), ('v', 6, 2),
          ('v', 4, 2), ('v', 3, 1), ('v', 2, 1), ('v', 1, 1), ('v', 0, 1)]
_N_EARLY = 5
_HEAD = 2
_X_SPLIT = 2

_X_ORDER = [
    [0, 1, 2, 3, 4, 5, 6, 7, 8, 9, 10, 11, 12, 13, 14, 15],
    [0, 1, 2, 3, 4, 10, 5, 11, 6, 12, 7, 13, 8, 14, 9, 15],
    [0, 5, 1, 6, 2, 7, 3, 8, 4, 9, 10, 13, 11, 14, 12, 15],
    [5, 6, 7, 8, 9, 13, 0, 14, 1, 15, 2, 10, 3, 11, 4, 12],
]
_X_SENDS = [
    [[(0, 0), (5, 1), (1, 0), (6, 1), (2, 0), (7, 1), (3, 0), (8, 1), (4, 0), (9, 1), (10, 0), (13,
     1), (11, 0), (14, 1), (12, 0), (15, 1), (13, 0), (10, 1), (14, 0), (11, 1), (15, 0), (12, 1)],
     [], [], [], [], [], []],
    [[(0, 0), (1, 0), (2, 0), (3, 0)], [(4, 0), (10, 0)], [(11, 0)], [(12, 0)], [], [], []],
    [[(5, 1), (0, 0), (6, 1), (1, 0)], [(7, 1), (2, 0)], [(8, 1), (3, 0), (9, 1), (4, 0)], [], [],
     [], []],
    [[(5, 1), (6, 1), (7, 1), (8, 1)], [(9, 1), (13, 1)], [(14, 1)], [(15, 1)], [], [], []],
]

_STEPS = [
    (4, 2, [('q', 0, 3, 0, 64), ('k', 0, 3, 0, 64)]),
    (6, 2, [('ld', 5, 12)]),
    (8, 3, [('q', 0, 3, 64, 128), ('k', 0, 3, 64, 128), ('q', 3, 3, 0, 128)]),
    (8, 3, [('ldo',)]),
    (12, 3, [('q', 0, 6, 128, 192), ('k', 0, 3, 128, 192)]),
    (12, 4, [('k', 3, 3, 0, 192)]),
    (16, 4, [('q', 0, 6, 192, 256), ('k', 0, 6, 192, 256)]),
    (16, 5, [('sm', 0, 4), ('q', 6, 2, 0, 256)]),
    (16, 6, [('sm', 4, 6), ('k', 6, 2, 0, 256)]),
    (16, 7, [('sm', 6, 8), ('v', 6, 2, 0, 256)]),
    (16, 8, [('pv', 6, 7), ('v', 4, 2, 0, 256)]),
    (16, 9, [('pv', 4, 5), ('v', 3, 1, 0, 256)]),
    (16, 10, [('v', 2, 1, 0, 256)]),
    (16, 11, [('pv', 3, 2), ('v', 1, 1, 0, 256)]),
    (16, 12, [('v', 0, 1, 0, 256), ('pv', 1, 0)]),
]

_AR_ROWS = [80, 64, 80, 32, 64, 64, 48, 80, 64, 64, 64, 64, 64, 48, 80, 64, 64, 64, 64, 64, 48, 48,
            48, 112, 64, 64, 64, 64, 64, 64, 64, 64]
_AR_PROG = [
    (
        "m2.8.8 s10.0.0 s11.1.0 m2.0.8 s9.1.0 s8.1.0 m0.0.6 s0.0.0 m0.6.10 s3.0.0 s1.0.0 m6.0.6 "
        "s24.1.0 s2.0.0 m6.6.10 s25.1.1 s26.1.1 m3.0.6 s12.0.0 m3.6.10 s13.0.0 s27.1.1 s15.0.0 m4.0.6 "
        "s16.1.1 m4.6.10 s19.1.0 s18.1.0 s14.0.1 m1.0.6 s4.0.1 s17.1.0 m1.6.10 s7.0.0 s5.0.0 m7.10.6 "
        "s31.1.1 m7.0.10 s25.0.1 s29.1.0 s30.1.0 m5.10.6 s24.0.1 s28.1.0 m5.0.10 s21.0.1 s21.1.1 "
        "s23.0.1 s22.1.1 s23.1.1 f21.1.3 f20.1.3 f22.1.3 f27.1.3 f23.1.3 f25.1.3 f24.1.1 f4.1.3 "
        "s16.0.1 s22.0.1 s20.1.1 s6.0.1 f26.1.3 f7.1.2 f19.1.1 f5.1.2 s14.1.1 s20.0.1 f16.1.3 f6.1.3 "
        "f18.1.1 f12.1.2 s31.0.1 s4.1.1 s26.0.1 s6.1.1 f17.1.1 f14.1.3 s0.1.1 s27.0.1 f31.1.3 f13.1.2 "
        "f29.1.1 f15.1.2 s28.0.1 s15.1.1 f30.1.1 f0.1.2 f28.1.1 f1.1.2 f11.1.1 f2.1.2 f8.1.1 f3.1.2 "
        "f9.1.1 f10.1.2 "
    ),
    (
        "m6.0.8 s25.1.0 s24.0.0 m6.8.8 s26.1.0 s27.1.0 m4.0.6 s16.1.0 m4.6.10 s19.0.0 s18.0.0 m5.0.6 "
        "s20.1.0 s17.0.0 m5.6.10 s22.1.0 m7.0.6 s21.1.1 s28.0.0 m7.6.10 s29.0.0 s31.1.0 s30.0.0 "
        "m2.10.6 s23.1.1 s11.0.0 m2.0.10 s10.0.1 m1.0.6 s8.0.0 s4.1.1 m1.6.10 s9.0.0 s7.1.1 m3.0.6 "
        "s5.1.1 s12.0.1 m3.6.10 s6.1.1 s13.0.1 m0.0.6 s0.0.1 s12.1.1 m0.6.10 f12.1.3 s14.1.1 s3.0.1 "
        "s13.1.1 s7.0.1 f4.1.3 f14.1.3 s15.1.1 s2.0.1 f13.1.3 f7.1.3 s0.1.1 s1.0.1 f15.1.3 f5.1.3 "
        "s1.1.1 s5.0.1 f25.1.1 f0.1.3 s2.1.1 s21.0.1 f24.0.1 f1.1.3 s3.1.1 s14.0.1 f21.1.3 s10.1.1 "
        "s23.0.1 s4.0.1 f2.1.3 f3.1.3 s6.0.1 s15.0.1 f23.1.3 f10.1.3 f16.1.1 f8.1.2 f22.1.1 f19.1.2 "
        "f6.1.3 f20.1.1 f18.1.2 f31.1.1 f9.1.2 f26.1.1 f11.1.2 f27.1.1 f29.1.2 f28.0.1 f30.1.2 "
        "f17.1.2 "
    ),
    (
        "m5.0.8 s21.1.0 s20.0.0 m5.8.8 s22.0.0 s23.1.0 m6.10.6 s27.0.0 m6.0.10 s25.0.0 s24.0.1 m1.0.6 "
        "s4.1.0 s26.0.0 m1.6.10 s7.1.1 s5.1.1 m4.10.6 s19.0.1 s6.1.0 m4.0.10 s16.0.0 s18.0.1 m3.0.6 "
        "s12.1.1 s17.0.1 m3.6.10 s14.1.0 s13.1.1 m7.10.6 s31.0.0 s15.1.1 m7.0.10 s29.0.1 s30.0.1 "
        "m0.0.6 s0.1.1 s28.0.1 m0.6.10 s1.1.1 s2.1.1 m2.10.6 s11.0.1 m2.0.10 s8.0.1 s3.1.1 f25.1.2 "
        "s10.1.1 s9.0.1 s8.1.1 f8.1.3 s12.0.1 s19.1.1 s10.0.1 f10.1.3 f12.1.3 f16.1.2 f13.1.3 s18.1.1 "
        "s3.0.1 s13.0.1 f19.1.3 s9.1.1 s7.0.1 f0.1.3 f3.1.3 f18.1.3 s11.1.1 f9.1.3 f7.1.3 s2.0.1 "
        "s29.1.1 f11.1.3 s1.0.1 f2.1.3 s30.1.1 f29.1.3 s5.0.1 f1.1.3 s17.1.1 f30.1.3 f5.1.3 f17.1.3 "
        "f21.1.1 f22.1.2 f14.1.1 f24.1.3 f27.1.2 f23.1.1 f28.1.3 f4.1.1 f31.1.2 f6.1.1 f26.1.2 "
        "f15.1.3 f20.1.2 "
    ),
    (
        "m1.0.8 s5.1.0 s4.0.0 m1.8.8 s7.1.0 s6.0.0 m5.0.6 s21.0.0 m5.6.10 s23.0.0 m3.0.6 s12.1.0 "
        "m3.6.10 s14.0.0 s13.1.0 s15.1.0 m0.0.6 s0.1.0 s20.0.1 m0.6.10 s3.1.0 s22.0.1 s2.1.0 m6.10.6 "
        "s27.0.1 m6.0.10 s25.0.1 s1.1.0 m2.0.6 s25.1.1 s24.0.1 m2.6.10 s8.1.1 s26.0.1 m4.10.6 s19.0.1 "
        "s10.1.0 m4.0.10 s16.0.1 s16.1.1 m7.0.6 s19.1.1 s18.0.1 m7.6.10 s17.0.1 s18.1.1 f25.1.3 "
        "f24.1.3 f26.1.3 f27.1.3 f16.1.3 f19.1.3 s31.0.1 s9.1.1 f18.1.3 s29.0.1 s11.1.1 f17.1.3 "
        "s30.0.1 s29.1.1 f31.1.3 s28.0.1 s30.1.1 f29.1.3 s11.0.1 s17.1.1 f30.1.3 s8.0.1 f28.1.3 "
        "s22.1.1 f11.1.3 s9.0.1 s24.1.1 s27.1.1 s28.1.1 s31.1.1 s26.1.1 f21.1.2 f8.1.3 f22.1.3 "
        "s20.1.1 f9.1.3 f23.1.2 f12.1.1 f20.1.3 f10.1.1 f3.1.1 f14.1.2 f13.1.1 f4.1.2 f7.1.1 f6.1.2 "
        "f2.1.1 f0.0.2 f1.1.1 f15.0.2 f5.1.1 "
    ),
]


def _w_dmas():
    out, sem = [], 0
    for i, (_, h0, nh) in enumerate(_LOADS):
        if nh < 3:
            parts = [(0, 32, half, h * DH, DH) for h in range(h0, h0 + nh) for half in range(2)]
        elif i == 0:
            parts = [(0, _HEAD, None, h0 * DH, nh * DH), (_HEAD, 32 - _HEAD, None, h0 * DH, nh * DH)]
        else:
            parts = [(0, 32, None, h0 * DH, nh * DH)]
        out.append([p + (sem + n,) for n, p in enumerate(parts)])
        sem += len(parts)
    return out, sem


def _x_ops(d):
    per_part = SEQ // PIECE // _X_SPLIT
    have = set(range(per_part)) if d == 0 else set()
    steps = []
    for sends, (n_pieces, _, _) in zip(_X_SENDS[d], _STEPS):
        ops = []
        for p, direction in sends + [(p, None) for p in _X_ORDER[d][:n_pieces]]:
            if p not in have:
                if d == 0:
                    ops.append(("cvt", p // per_part))
                    have.update(range(p // per_part * per_part, (p // per_part + 1) * per_part))
                else:
                    ops.append(("recv", p))
                    have.add(p)
            if direction is not None:
                ops.append(("send", p, direction))
        steps.append(ops)
    return steps


def _ar_ops(d):
    prog = [(op[0],) + tuple(int(v) for v in op[1:].split(".")) for op in _AR_PROG[d].split()]
    slots = [op[1:] for op in prog if op[0] == "m"]
    order = list(dict.fromkeys(s[0] for s in slots))
    last_send = max(i for i, op in enumerate(prog) if op[0] == "s")
    segs, arrived, in_flight, n_blocks = [], set(), [], 0

    def drain(keep):
        while len(in_flight) > keep:
            segs[-1].append(("sent",) + in_flight.pop(0))

    for i, (kind, u, p0, p1) in enumerate(prog):
        if kind == "m":
            if order.index(u) == n_blocks:
                if segs:
                    segs[-1].append(("wo", u, n_blocks))
                n_blocks += 1
            segs.append([])
            continue
        if i == len(prog) - 2:
            drain(2)
        for direction in range(2):
            needed = (p1 and p0 == direction) if kind == "s" else p1 >> direction & 1
            if needed and (u, direction) not in arrived:
                segs[-1].append(("recv", u, direction))
                arrived.add((u, direction))
        segs[-1].append((kind, u, p0, p1))
        if kind == "s":
            in_flight.append((u, p0, p1))
        if i == last_send:
            segs[-1] += [("xsent", p, direction) for sends in _X_SENDS[d] for p, direction in sends]
            drain(16)
    drain(0)
    return slots, order, segs


_W_DMAS, _N_WSEM = _w_dmas()
_X_OPS = [_x_ops(d) for d in range(N_DEV)]
_SLOTS, _WO_ORDER, _AR_OPS = zip(*[_ar_ops(d) for d in range(N_DEV)])
_N_UNITS = len(_AR_ROWS)
_ROW0 = [sum(_AR_ROWS[u // UNITS * UNITS:u]) for u in range(_N_UNITS)]


def _neighbour(d, direction):
    return (d + (1, N_DEV - 1)[direction]) % N_DEV


def _cols(h0, nh=1):
    return slice(h0 * DH, (h0 + nh) * DH)


def _body(x_hbm, wq_hbm, wk_hbm, wv_hbm, wo_hbm, out_ref,
          xf, wq, wk, wv, wo, xb, qb, kb, vb, pb, ab,
          acc, own_bf, sbuf, rbuf, lsem, ssem, rsem, xssem, xrsem):
    w_hbm = dict(q=wq_hbm, k=wk_hbm, v=wv_hbm)
    w_buf = dict(q=wq, k=wk, v=wv)
    x_rows = SEQ // _X_SPLIT

    def w_copy(i, n):
        g0, groups, half, c0, cols, sem = _W_DMAS[i][n]
        idx = (pl.ds(g0, groups), ALL if half is None else half, ALL, pl.ds(c0, cols))
        w = _LOADS[i][0]
        return pltpu.make_async_copy(w_hbm[w].at[idx], w_buf[w].at[idx], lsem.at[sem])

    def x_copy(i):
        rows = pl.ds(i * x_rows, x_rows)
        return pltpu.make_async_copy(x_hbm.at[0, rows], xf.at[rows], lsem.at[_N_WSEM + 16 + i])

    def wo_copy(b, k, half):
        return pltpu.make_async_copy(wo_hbm.at[:, half, :, pl.ds(times(b, DH), DH)],
                                     wo.at[b, :, half], lsem.at[_N_WSEM + 2 * k + half])

    w_copy(0, 0).start()

    me = lax.axis_index("i")

    def pick(vals):
        if len(set(vals)) == 1:
            return vals[0]
        packed = sum(v << (4 * d) for d, v in enumerate(vals))
        return (packed >> (4 * me)) & 15

    def times(v, m):
        return v * m if isinstance(v, int) else pl.multiple_of(v * m, m)

    def per_chip(emit, ops):
        for d in range(N_DEV):
            if ops[d]:
                pl.when(me == d)(functools.partial(emit, d, ops[d]))

    barrier = pltpu.get_barrier_semaphore()
    for nbr in (me ^ 1, me ^ 3):
        pl.semaphore_signal(barrier, inc=1, device_id=(nbr,), device_id_type=MESH)

    @pl.when(me == 0)
    def _():
        for i in range(_X_SPLIT):
            x_copy(i).start()

    for i in range(_N_EARLY):
        for n in range(i == 0, len(_W_DMAS[i])):
            w_copy(i, n).start()

    def project(w, h0, nh, r0, r1):
        wt = w_buf[w][:, :, :, _cols(h0, nh)].reshape(D, nh * DH).astype(BF16)
        r = jnp.dot(xb[r0:r1, :], wt, preferred_element_type=F32)
        if w == "q":
            r = (r * SCALE).astype(BF16)
            for p in range(r0 // PIECE, r1 // PIECE):
                g = pick([_X_ORDER[d][p] for d in range(N_DEV)])
                qb[pl.ds(times(g, PIECE), PIECE), _cols(h0, nh)] = r[p * PIECE - r0:(p + 1) * PIECE - r0]
        else:
            (kb if w == "k" else vb)[r0:r1, _cols(h0, nh)] = r.astype(BF16)

    def softmax(h):
        s = lax.dot_general(qb[:, _cols(h)], kb[:, _cols(h)], (((1,), (1,)), ((), ())),
                            preferred_element_type=F32)
        e = jnp.exp(s - jnp.max(s, axis=-1, keepdims=True))
        pb[h] = (e * (1.0 / jnp.sum(e, axis=-1, keepdims=True))).astype(BF16)

    def run(job):
        if job[0] in ("q", "k", "v"):
            project(*job)
        elif job[0] == "sm":
            for h in range(job[1], job[2]):
                softmax(h)
        elif job[0] == "pv":
            for h in job[1:]:
                ab[:, _cols(h)] = jnp.dot(pb[h], vb[:, _cols(h)], preferred_element_type=F32).astype(BF16)
        elif job[0] == "ld":
            for i in range(job[1], job[2]):
                for n in range(len(_W_DMAS[i])):
                    w_copy(i, n).start()
        else:
            for k in range(8):
                b = pick([_WO_ORDER[d][k] for d in range(N_DEV)])
                for half in range(2):
                    wo_copy(b, k, half).start()

    def wait_recv(d, dst, send_sem, recv_sem):
        pltpu.make_async_remote_copy(dst, dst, send_sem, recv_sem, device_id=(d,),
                                     device_id_type=MESH).wait_recv()

    def x_piece(d, p):
        return xb.at[pl.ds(_X_ORDER[d].index(p) * PIECE, PIECE)]

    def x_hop(d, p, direction):
        t = _neighbour(d, direction)
        return pltpu.make_async_remote_copy(x_piece(d, p), x_piece(t, p), xssem.at[direction * 16 + p],
                                            xrsem.at[p], device_id=(t,), device_id_type=MESH)

    def x_emit(d, ops):
        for kind, p, *direction in ops:
            if kind == "cvt":
                x_copy(p).wait()
                xb[p * x_rows:(p + 1) * x_rows, :] = xf[p * x_rows:(p + 1) * x_rows, :].astype(BF16)
            elif kind == "recv":
                wait_recv(d, x_piece(d, p), xssem.at[p], xrsem.at[p])
            else:
                x_hop(d, p, *direction).start()

    pl.when(me == 0)(functools.partial(x_emit, 0, [("cvt", 0)]))
    pl.semaphore_wait(barrier, 2)

    n_waited = 0
    for j, (_, n_loads, jobs) in enumerate(_STEPS):
        if j < len(_X_OPS[0]):
            per_chip(x_emit, [_X_OPS[d][j] for d in range(N_DEV)])
        for i in range(n_waited, n_loads):
            for n in range(len(_W_DMAS[i])):
                w_copy(i, n).wait()
        n_waited = n_loads
        for job in jobs:
            run(job)

    def hop(d, u, direction, add):
        b, rows = u // UNITS, pl.ds(_ROW0[u], _AR_ROWS[u])
        src = sbuf.at[direction, b, rows] if add else own_bf.at[b, rows]
        sem = direction * _N_UNITS + u
        return pltpu.make_async_remote_copy(src, rbuf.at[direction, b, rows], ssem.at[sem], rsem.at[sem],
                                            device_id=(_neighbour(d, direction),), device_id_type=MESH)

    def ar_emit(d, ops):
        for kind, u, *args in ops:
            if kind == "sent":
                hop(d, u, *args).wait_send()
            elif kind == "xsent":
                x_hop(d, u, *args).wait_send()
            elif kind == "wo":
                for half in range(2):
                    wo_copy(u, *args, half).wait()
            else:
                b, rows = u // UNITS, pl.ds(_ROW0[u], _AR_ROWS[u])
                if kind == "recv":
                    sem = args[0] * _N_UNITS + u
                    wait_recv(d, rbuf.at[args[0], b, rows], ssem.at[sem], rsem.at[sem])
                elif kind == "s":
                    direction, add = args
                    if add:
                        total = rbuf[direction, b, rows].astype(F32) + acc[b, rows]
                        sbuf[direction, b, rows] = total.astype(BF16)
                    hop(d, u, direction, add).start()
                else:
                    own, mask = args
                    terms = [rbuf[k, b, rows].astype(F32) for k in range(2) if mask >> k & 1]
                    terms += [acc[b, rows]] if own else []
                    out_ref[0, rows, _cols(b)] = sum(terms[1:], terms[0])

    for half in range(2):
        wo_copy(pick([_WO_ORDER[d][0] for d in range(N_DEV)]), 0, half).wait()
    for j, (_, _, pieces) in enumerate(_SLOTS[0]):
        b = pick([_SLOTS[d][j][0] for d in range(N_DEV)])
        rows = pl.ds(times(pick([_SLOTS[d][j][1] for d in range(N_DEV)]), PIECE), pieces * PIECE)
        part = jnp.dot(ab[rows, :], wo[b].reshape(D, DH).astype(BF16), preferred_element_type=F32)
        acc[b, rows] = part
        own_bf[b, rows] = part.astype(BF16)
        per_chip(ar_emit, [_AR_OPS[d][j] for d in range(N_DEV)])


def pallas_dist_attn_self_mha_htp_b1_sq256_skv256_d1024_hq8_dh128_kernel(
    x: jax.Array,
    Wq: jax.Array,
    Wk: jax.Array,
    Wv: jax.Array,
    Wo: jax.Array,
):
    vmem, dma = pltpu.VMEM, pltpu.SemaphoreType.DMA
    view = (32, 2, 16, D)
    act = vmem((SEQ, D), BF16)
    return pl.pallas_call(
        _body,
        out_shape=jax.ShapeDtypeStruct(x.shape, F32),
        in_specs=[pl.BlockSpec(memory_space=pl.ANY)] * 5,
        out_specs=pl.BlockSpec(memory_space=pltpu.VMEM),
        scratch_shapes=[
            vmem((SEQ, D), F32),
            vmem(view, F32), vmem(view, F32), vmem(view, F32),
            vmem((8, 32, 2, 16, DH), F32),
            act, act, act, act,
            vmem((8, SEQ, SEQ), BF16), act,
            vmem((8, SEQ, DH), F32), vmem((8, SEQ, DH), BF16),
            vmem((2, 8, SEQ, DH), BF16), vmem((2, 8, SEQ, DH), BF16),
            dma((_N_WSEM + 16 + _X_SPLIT,)), dma((2 * _N_UNITS,)), dma((2 * _N_UNITS,)),
            dma((32,)), dma((16,)),
        ],
        compiler_params=pltpu.CompilerParams(
            collective_id=0,
            vmem_limit_bytes=64 * 1024 * 1024,
            disable_semaphore_checks=True,
        ),
    )(x, Wq.reshape(view), Wk.reshape(view), Wv.reshape(view), Wo.reshape(view))
```
